```python
import numpy as np

kernel_name = "dist_ring_attn_i_s256_d64"

def setup_inputs():
    S, D = 1024, 64
    q = np.random.randn(S, D).astype(np.float32)
    k = np.random.randn(S, D).astype(np.float32)
    v = np.random.randn(S, D).astype(np.float32)
    return {"q": q, "k": k, "v": v}

def reference(q: np.ndarray, k: np.ndarray, v: np.ndarray) -> np.ndarray:
    D = q.shape[1]
    scores = q @ k.T / np.sqrt(D)
    scores_max = np.max(scores, axis=1, keepdims=True)
    weights = np.exp(scores - scores_max)
    weights = weights / np.sum(weights, axis=1, keepdims=True)
    return weights @ v
```

```python
import functools
import math
import jax
import jax.numpy as jnp
from jax import lax
from jax.experimental import pallas as pl
from jax.experimental.pallas import tpu as pltpu

N = 4
S, D = 256, 64
H = 128
MESH = pl.DeviceIdType.MESH
LOG2E = 1.4426950408889634
BF = jnp.bfloat16

PIECE = {
    "K": ("k", None, None), "K0": ("k", 0, None), "K1": ("k", 1, None),
    "V": ("v", None, None), "V0": ("v", 0, None), "V1": ("v", 1, None),
    "V0a": ("v", 0, 0), "V0b": ("v", 0, 32), "V1a": ("v", 1, 0), "V1b": ("v", 1, 32),
    "K0a": ("k", 0, 0), "K0b": ("k", 0, 32), "K1a": ("k", 1, 0), "K1b": ("k", 1, 32),
}
LOAD = {"K": (0, None), "V": (1, None), "Q": (2, None), "K0": (0, 0), "K1": (0, 1), "V0": (1, 0), "V1": (1, 1)}


def make(prog, cp=None):
    ridx = {p: {} for p in range(N)}
    lidx = {p: {} for p in range(N)}
    for p in range(N):
        for op in prog[p]:
            if op[0] == "wait":
                ridx[p].setdefault((op[1], op[2]), len(ridx[p]))
            if op[0] == "ld":
                lidx[p].setdefault(op[1], len(lidx[p]))
    nrecv = max(len(ridx[p]) for p in range(N))
    nld = max(len(lidx[p]) for p in range(N))
    sent = {p: set() for p in range(N)}
    for p in range(N):
        for op in prog[p]:
            if op[0] == "send":
                _, piece, sslot, t = op
                dslot = ((p + sslot) % N - t) % N
                assert (piece, dslot) in ridx[t], (p, op)
                assert (piece, dslot) not in sent[t], (p, op)
                sent[t].add((piece, dslot))
    for p in range(N):
        assert sent[p] == set(ridx[p]), (p, sent[p] ^ set(ridx[p]))

    def f(q, k, v):
        def body(q_hbm, k_hbm, v_hbm, o_ref, in_buf, k_buf, v_buf, ld_sems, send_sem, recv_sems, go_sem):
            me = lax.axis_index("i")
            barrier = pltpu.get_barrier_semaphore()
            hbm = (k_hbm, v_hbm, q_hbm)

            def view(piece, slot):
                b, h, r = PIECE[piece]
                ref = (k_buf if b == "k" else v_buf).at[slot]
                if h is not None:
                    ref = ref.at[h]
                    if r is not None:
                        ref = ref.at[pl.ds(r, 32)]
                return ref

            def run(p):
                def load_desc(name):
                    a, h = LOAD[name]
                    src, dst = hbm[a], in_buf.at[a]
                    if h is not None:
                        src, dst = src.at[:, pl.ds(h * H, H)], dst.at[:, pl.ds(h * H, H)]
                    return pltpu.make_async_copy(src, dst, ld_sems.at[lidx[p][name]])

                def send_desc(op):
                    _, piece, sslot, t = op
                    dslot = ((p + sslot) % N - t) % N
                    return pltpu.make_async_remote_copy(
                        src_ref=view(piece, sslot), dst_ref=view(piece, dslot),
                        send_sem=send_sem, recv_sem=recv_sems.at[ridx[t][(piece, dslot)]],
                        device_id=(t,), device_id_type=MESH)

                st = {}
                qs = None
                M = L = acc = None
                beta = {}
                for n, op in enumerate(prog[p]):
                    kind = op[0]
                    if True:
                        if kind == "ld":
                            load_desc(op[1]).start()
                        elif kind == "cast":
                            load_desc(op[1]).wait()
                            a, h = LOAD[op[1]]
                            if a == 2:
                                qs = (in_buf[2] * (LOG2E / math.sqrt(D))).astype(BF)
                            else:
                                dst = k_buf if a == 0 else v_buf
                                for hh in ((0, 1) if h is None else (h,)):
                                    dst[0, hh] = in_buf[a, :, hh * H:(hh + 1) * H].astype(BF)
                        elif kind == "barsig":
                            for t in op[1]:
                                pl.semaphore_signal(barrier, inc=1, device_id=(t,), device_id_type=MESH)
                        elif kind == "barwait":
                            pl.semaphore_wait(barrier, op[1])
                        elif kind == "gosig":
                            for t in op[1]:
                                pl.semaphore_signal(go_sem, inc=1, device_id=(t,), device_id_type=MESH)
                        elif kind == "gowait":
                            pl.semaphore_wait(go_sem, 1)
                        elif kind == "send":
                            send_desc(op).start()
                        elif kind == "wait":
                            _, piece, slot = op
                            pltpu.make_async_remote_copy(
                                src_ref=view(piece, slot), dst_ref=view(piece, slot),
                                send_sem=send_sem, recv_sem=recv_sems.at[ridx[p][(piece, slot)]],
                                device_id=(p,), device_id_type=MESH).wait_recv()
                        elif kind == "k":
                            _, slot, h = op
                            s = lax.dot_general(k_buf[slot, h], qs, (((0,), (0,)), ((), ())), preferred_element_type=jnp.float32)
                            m = jnp.max(s, axis=0, keepdims=True)
                            pp = jnp.exp2(s - m)
                            l = jnp.sum(pp, axis=0, keepdims=True)
                            st[(slot, h)] = (m, l, pp.astype(BF))
                        elif kind == "coef":
                            _, keys, final = op
                            Mn = functools.reduce(jnp.maximum, [st[key][0] for key in keys] + ([M] if M is not None else []))
                            for key in keys:
                                beta[key] = jnp.exp2(st[key][0] - Mn)
                            Ln = functools.reduce(lambda a_, b_: a_ + b_, [st[key][1] * beta[key] for key in keys])
                            if M is not None:
                                al = jnp.exp2(M - Mn)
                                Ln = Ln + L * al
                            M, L = Mn, Ln
                            if final:
                                inv = 1.0 / L
                                for key in keys:
                                    beta[key] = beta[key] * inv
                                if acc is not None:
                                    al = al * inv
                            if acc is not None:
                                acc = acc * al
                        elif kind == "pv":
                            _, slot, h = op
                            t_ = jnp.dot(v_buf[slot, h], st[(slot, h)][2], preferred_element_type=jnp.float32) * beta[(slot, h)]
                            acc = t_ if acc is None else acc + t_
                        elif kind == "store":
                            o_ref[...] = acc
                        else:
                            raise ValueError(op)
                if True:
                    for op in prog[p]:
                        if op[0] == "send":
                            send_desc(op).wait_send()

            for p in range(N):
                @pl.when(me == p)
                def _():
                    run(p)

        o = pl.pallas_call(
            body,
            out_shape=jax.ShapeDtypeStruct((D, S), jnp.float32),
            in_specs=[pl.BlockSpec(memory_space=pltpu.HBM)] * 3,
            out_specs=pl.BlockSpec(memory_space=pltpu.VMEM),
            scratch_shapes=[
                pltpu.VMEM((3, D, S), jnp.float32),
                pltpu.VMEM((N, 2, D, H), BF),
                pltpu.VMEM((N, 2, D, H), BF),
                pltpu.SemaphoreType.DMA((nld,)),
                pltpu.SemaphoreType.DMA,
                pltpu.SemaphoreType.DMA((nrecv,)),
                pltpu.SemaphoreType.REGULAR,
            ],
            compiler_params=pltpu.CompilerParams(collective_id=0, disable_semaphore_checks=True, **(cp or {})),
        )(q.T, k.T, v.T)
        return o.T
    return f


def blockK(slot):
    return [("k", slot, 0), ("k", slot, 1)]

def blockV(slot, final=False):
    return [("coef", ((slot, 0), (slot, 1)), final), ("pv", slot, 0), ("pv", slot, 1)]

OWN = [("cast", "Q")] + blockK(0) + blockV(0)

def prog(hold="V1b", y=24, c_first="V1", b_trigger="K3"):
    P = {}
    a = [("ld", "K"), ("ld", "V"), ("ld", "Q"), ("barsig", (1, 3, 2)),
         ("cast", "K"), ("barwait", 2), ("send", "K", 0, 3), ("send", "K", 0, 1),
         ("cast", "V"), ("send", "V", 0, 3), ("send", "V", 0, 1)] + OWN + \
        [("gowait",), ("send", "K", 0, 2), ("send", "V", 0, 2),
         ("wait", "K", 3), ("send", "K", 3, 1)] + blockK(3) + \
        [("wait", "K", 1)] + blockK(1) + \
        [("wait", "V", 3), ("send", "V", 3, 1)] + blockV(3)
    if hold == "none":
        a += [("wait", "V", 1)] + blockV(1)
        fin = ((2, 0), (2, 1))
        lateB = []
    else:
        a += [("wait", "V0", 1), ("coef", ((1, 0),), False), ("pv", 1, 0)]
        fin = ((1, 1), (2, 0), (2, 1))
        lateB = ([("wait", "V1", 1)] if hold == "V1" else [("wait", "V1a", 1), ("wait", "V1b", 1)])
    a += [("wait", "K", 2)] + blockK(2) + [("coef", fin, True),
          ("wait", "V1a", 2), ("wait", "V1b", 2)] + lateB
    if y == 24:
        a += [("wait", "V0a", 2), ("wait", "V0b", 2)]
    elif y == 16:
        a += [("wait", "V0", 2)]
    elif y == 32:
        a += [("wait", "V0a", 2), ("wait", "V0b", 2)]
    a += [("pv", 2, 1), ("pv", 2, 0)] + ([("pv", 1, 1)] if hold != "none" else []) + [("store",)]
    P[0] = a
    b = [("ld", "K"), ("ld", "V"), ("ld", "Q"), ("barsig", (0, 2)),
         ("cast", "K"), ("barwait", 1), ("send", "K", 0, 0), ("cast", "V")]
    if hold == "none":
        b += [("send", "V", 0, 0)]; held = []
    elif hold == "V1":
        b += [("send", "V0", 0, 0)]; held = [("send", "V1", 0, 0)]
    else:
        b += [("send", "V0", 0, 0), ("send", "V1a", 0, 0)]; held = [("send", "V1b", 0, 0)]
    b += OWN + [("gowait",), ("send", "K", 0, 3), ("send", "V", 0, 3), ("send", "K", 0, 2), ("send", "V", 0, 2)]
    if b_trigger == "go":
        b += held
    b += [("wait", "K", 3)]
    if b_trigger == "K3":
        b += held
    b += blockK(3) + [("wait", "V", 3)] + blockV(3) + \
         [("wait", "K", 1)] + blockK(1) + [("wait", "K", 2)] + blockK(2) + \
         [("wait", "V", 1)] + blockV(1) + [("coef", ((2, 0), (2, 1)), True), ("wait", "V", 2), ("pv", 2, 0), ("pv", 2, 1), ("store",)]
    P[1] = b
    if c_first == "V1":
        c = [("ld", "V1"), ("ld", "K"), ("ld", "V0"), ("ld", "Q"), ("barwait", 3), ("gosig", (1, 3, 0)),
             ("cast", "V1"), ("send", "V1a", 0, 3), ("send", "V1b", 0, 3), ("cast", "K"), ("send", "K", 0, 0), ("cast", "V0")]
    else:
        c = [("ld", "K"), ("ld", "V1"), ("ld", "V0"), ("ld", "Q"), ("barwait", 3), ("gosig", (1, 3, 0)),
             ("cast", "K"), ("send", "K", 0, 0), ("cast", "V1"), ("send", "V1a", 0, 3), ("send", "V1b", 0, 3), ("cast", "V0")]
    if y == 24:
        c += [("send", "V0b", 0, 3), ("send", "V0a", 0, 0), ("send", "K", 0, 3), ("send", "V0a", 0, 3)]
    elif y == 16:
        c += [("send", "V0", 0, 0), ("send", "K", 0, 3), ("send", "V0", 0, 3)]
    elif y == 32:
        c += [("send", "V0b", 0, 3), ("send", "V0a", 0, 3), ("send", "K", 0, 3)]
    c += [("send", "K", 0, 1), ("send", "V", 0, 1)] + OWN + \
         [("wait", "K", 1)] + blockK(1) + [("wait", "V", 1)] + blockV(1) + \
         [("wait", "K", 2)] + blockK(2) + [("wait", "K", 3)] + blockK(3) + \
         [("wait", "V", 2)] + blockV(2) + [("coef", ((3, 0), (3, 1)), True), ("wait", "V", 3), ("pv", 3, 0), ("pv", 3, 1), ("store",)]
    P[2] = c
    d = [("ld", "K"), ("ld", "V"), ("ld", "Q"), ("barsig", (0, 2)),
         ("cast", "K"), ("barwait", 1), ("send", "K", 0, 0),
         ("cast", "V"), ("send", "V", 0, 0)] + OWN + \
        [("gowait",), ("send", "K", 0, 2), ("send", "V", 0, 2),
         ("wait", "V1a", 3), ("send", "V1a", 3, 0), ("wait", "V1b", 3), ("send", "V1b", 3, 0)]
    if y == 24:
        d += [("wait", "V0b", 3), ("send", "V0b", 3, 0)]; v0w = [("wait", "V0a", 3)]
    elif y == 16:
        v0w = [("wait", "V0", 3)]
    elif y == 32:
        d += [("wait", "V0b", 3), ("send", "V0b", 3, 0), ("wait", "V0a", 3), ("send", "V0a", 3, 0)]; v0w = []
    d += [("wait", "K", 1)] + blockK(1) + [("wait", "K", 3)] + blockK(3) + \
         [("wait", "V", 1)] + blockV(1) + v0w + blockV(3) + \
         [("wait", "K", 2)] + blockK(2) + [("coef", ((2, 0), (2, 1)), True), ("wait", "V", 2), ("pv", 2, 0), ("pv", 2, 1), ("store",)]
    P[3] = d
    return P


def pallas_dist_ring_attn_i_s256_d64_kernel(q, k, v):
    return make(prog(hold="V1b", c_first="K", y=24))(q, k, v)
```

```python
import math

import jax
import jax.numpy as jnp
from jax import lax
from jax.experimental import pallas as pl
from jax.experimental.pallas import tpu as pltpu

N_DEV = 4
S_LOC = 256
D = 64
HALF = 128
_BF16 = jnp.bfloat16
_MESH = pl.DeviceIdType.MESH
_Q_SCALE = math.log2(math.e) / math.sqrt(D)

_LOADS = {
    "k": (0, None), "k0": (0, 0), "k1": (0, 1),
    "v": (1, None), "v0": (1, 0), "v1": (1, 1),
    "q": (2, None),
}

_PIECES = {
    "K": ("k", 0, 128), "K0": ("k", 0, 64), "K1": ("k", 64, 64),
    "V": ("v", 0, 128), "V0": ("v", 0, 64),
    "V0a": ("v", 0, 32), "V0b": ("v", 32, 32), "V1a": ("v", 64, 32), "V1b": ("v", 96, 32),
}


def _scores(block):
    return [("scores", block)]


def _values(*halves, last=False):
    return [("rescale", halves, last)] + [("pv",) + h for h in halves]


_PROGRAM = {
    0: (
        [("load", "k"), ("load", "v"), ("load", "q"), ("enter", (1, 3, 2)),
         ("use", "k"), ("entered", 2), ("send", "K", 0, 3), ("send", "K", 0, 1),
         ("use", "v"), ("send", "V", 0, 3), ("send", "V", 0, 1), ("use", "q")]
        + _scores(0) + _values((0, 0), (0, 1))
        + [("wait_go",), ("send", "K", 0, 2), ("send", "V", 0, 2),
           ("recv", "K", 3), ("send", "K", 3, 1), ("recv", "K0", 1), ("recv", "K1", 1)]
        + _scores(3) + _scores(1)
        + [("recv", "V", 3), ("send", "V", 3, 1), ("recv", "V0", 1)]
        + _values((3, 0), (3, 1), (1, 0))
        + [("recv", "K0", 2), ("recv", "K1", 2)]
        + _scores(2)
        + [("recv", "V1a", 2), ("recv", "V1b", 2), ("recv", "V1a", 1), ("recv", "V1b", 1),
           ("recv", "V0a", 2), ("recv", "V0b", 2)]
        + _values((2, 1), (2, 0), (1, 1), last=True)
        + [("store",)]
    ),
    1: (
        [("load", "k0"), ("load", "k1"), ("load", "v"), ("load", "q"), ("enter", (0, 2)),
         ("use", "k0"), ("entered", 1), ("send", "K0", 1, 0), ("use", "k1"), ("send", "K1", 1, 0),
         ("use", "v"), ("send", "V0", 1, 0), ("send", "V1a", 1, 0), ("use", "q")]
        + _scores(1) + _values((1, 0), (1, 1))
        + [("wait_go",), ("send", "K", 1, 3), ("send", "V", 1, 3), ("send", "K", 1, 2), ("send", "V", 1, 2),
           ("recv", "K", 0), ("send", "V1b", 1, 0)]
        + _scores(0) + [("recv", "V", 0)] + _values((0, 0), (0, 1))
        + [("recv", "K", 2)] + _scores(2) + [("recv", "K", 3)] + _scores(3)
        + [("recv", "V", 2)] + _values((2, 0), (2, 1))
        + [("recv", "V", 3)] + _values((3, 0), (3, 1), last=True)
        + [("store",)]
    ),
    2: (
        [("load", "v1"), ("load", "k0"), ("load", "k1"), ("load", "v0"), ("load", "q"),
         ("entered", 3), ("go", (1, 3, 0)),
         ("use", "v1"), ("send", "V1a", 2, 3), ("send", "V1b", 2, 3),
         ("use", "k0"), ("send", "K0", 2, 0), ("use", "k1"), ("send", "K1", 2, 0),
         ("use", "v0"), ("send", "V0b", 2, 3), ("send", "V0a", 2, 0),
         ("send", "K", 2, 3), ("send", "V0a", 2, 3), ("send", "K", 2, 1), ("send", "V", 2, 1), ("use", "q")]
        + _scores(2) + _values((2, 0), (2, 1))
        + [("recv", "K", 3)] + _scores(3) + [("recv", "V", 3)] + _values((3, 0), (3, 1))
        + [("recv", "K", 0)] + _scores(0) + [("recv", "K", 1)] + _scores(1)
        + [("recv", "V", 0)] + _values((0, 0), (0, 1))
        + [("recv", "V", 1)] + _values((1, 0), (1, 1), last=True)
        + [("store",)]
    ),
    3: (
        [("load", "k"), ("load", "v"), ("load", "q"), ("enter", (0, 2)),
         ("use", "k"), ("entered", 1), ("send", "K", 3, 0),
         ("use", "v"), ("send", "V", 3, 0), ("use", "q")]
        + _scores(3) + _values((3, 0), (3, 1))
        + [("wait_go",), ("send", "K", 3, 2), ("send", "V", 3, 2),
           ("recv", "V1a", 2), ("send", "V1a", 2, 0), ("recv", "V1b", 2), ("send", "V1b", 2, 0),
           ("recv", "V0b", 2), ("send", "V0b", 2, 0)]
        + [("recv", "K", 0)] + _scores(0) + [("recv", "K", 2)] + _scores(2)
        + [("recv", "V", 0)] + _values((0, 0), (0, 1))
        + [("recv", "V0a", 2)] + _values((2, 0), (2, 1))
        + [("recv", "K", 1)] + _scores(1)
        + [("recv", "V", 1)] + _values((1, 0), (1, 1), last=True)
        + [("store",)]
    ),
}


def _semaphore_plan():
    recv, loads = [], []
    for chip in range(N_DEV):
        steps = _PROGRAM[chip]
        recv.append({s[1:]: n for n, s in enumerate(s for s in steps if s[0] == "recv")})
        loads.append({s[1]: n for n, s in enumerate(s for s in steps if s[0] == "load")})
    sent = sorted(s[3:] + s[1:3] for chip in range(N_DEV) for s in _PROGRAM[chip] if s[0] == "send")
    received = sorted((chip,) + key for chip in range(N_DEV) for key in recv[chip])
    assert sent == received, "every remote copy needs exactly one matching wait"
    return recv, loads


_RECV_SEM, _LOAD_SEM = _semaphore_plan()


def _body(q_hbm, k_hbm, v_hbm, o_ref, f32_buf, k_buf, v_buf, load_sems, send_sem, recv_sems, go_sem):
    hbm = (k_hbm, v_hbm, q_hbm)
    barrier = pltpu.get_barrier_semaphore()

    def piece(name, block):
        which, start, size = _PIECES[name]
        ref = (k_buf if which == "k" else v_buf).at[block]
        return ref if size == 2 * D else ref.at[pl.ds(start, size)]

    def run(me):
        def load(name):
            arr, half = _LOADS[name]
            src, dst = hbm[arr], f32_buf.at[arr]
            if half is not None:
                cols = pl.ds(half * HALF, HALF)
                src, dst = src.at[:, cols], dst.at[:, cols]
            return pltpu.make_async_copy(src, dst, load_sems.at[_LOAD_SEM[me][name]])

        def remote(name, block, chip):
            return pltpu.make_async_remote_copy(
                src_ref=piece(name, block),
                dst_ref=piece(name, block),
                send_sem=send_sem,
                recv_sem=recv_sems.at[_RECV_SEM[chip][(name, block)]],
                device_id=(chip,),
                device_id_type=_MESH,
            )

        weights = None
        stats = {}
        scale = {}
        run_max = run_sum = acc = None
        for step in _PROGRAM[me]:
            kind = step[0]
            if kind == "load":
                load(step[1]).start()
            elif kind == "use":
                load(step[1]).wait()
                arr, half = _LOADS[step[1]]
                if arr == 2:
                    q_t = (f32_buf[2] * _Q_SCALE).astype(_BF16)
                    zero = jnp.zeros_like(q_t)
                    weights = (jnp.concatenate([q_t, zero], axis=0), jnp.concatenate([zero, q_t], axis=0))
                else:
                    dst = k_buf if arr == 0 else v_buf
                    for h in (0, 1) if half is None else (half,):
                        dst[me, h * D:(h + 1) * D] = f32_buf[arr, :, h * HALF:(h + 1) * HALF].astype(_BF16)
            elif kind == "enter":
                for chip in step[1]:
                    pl.semaphore_signal(barrier, inc=1, device_id=(chip,), device_id_type=_MESH)
            elif kind == "entered":
                pl.semaphore_wait(barrier, step[1])
            elif kind == "go":
                for chip in step[1]:
                    pl.semaphore_signal(go_sem, inc=1, device_id=(chip,), device_id_type=_MESH)
            elif kind == "wait_go":
                pl.semaphore_wait(go_sem, 1)
            elif kind == "send":
                remote(*step[1:]).start()
            elif kind == "recv":
                remote(step[1], step[2], me).wait_recv()
            elif kind == "scores":
                keys = k_buf[step[1]].T
                for half in (0, 1):
                    s_t = jnp.dot(keys, weights[half], preferred_element_type=jnp.float32)
                    row_max = jnp.max(s_t, axis=0, keepdims=True)
                    p_t = jnp.exp2(s_t - row_max)
                    stats[(step[1], half)] = (row_max, jnp.sum(p_t, axis=0, keepdims=True), p_t.astype(_BF16))
            elif kind == "rescale":
                halves, last = step[1:]
                new_max = run_max
                for h in halves:
                    new_max = stats[h][0] if new_max is None else jnp.maximum(new_max, stats[h][0])
                for h in halves:
                    scale[h] = jnp.exp2(stats[h][0] - new_max)
                new_sum = None
                for h in halves:
                    term = stats[h][1] * scale[h]
                    new_sum = term if new_sum is None else new_sum + term
                if run_max is not None:
                    keep = jnp.exp2(run_max - new_max)
                    new_sum = new_sum + run_sum * keep
                if last:
                    inv_sum = 1.0 / new_sum
                    keep = keep * inv_sum
                    for h in halves:
                        scale[h] = scale[h] * inv_sum
                if acc is not None:
                    acc = acc * keep
                run_max, run_sum = new_max, new_sum
            elif kind == "pv":
                h = step[1:]
                v_t = v_buf[h[0], h[1] * D:(h[1] + 1) * D]
                out = jnp.dot(v_t, stats[h][2], preferred_element_type=jnp.float32) * scale[h]
                acc = out if acc is None else acc + out
            elif kind == "store":
                o_ref[...] = acc
            else:
                raise ValueError(step)
        for step in _PROGRAM[me]:
            if step[0] == "send":
                remote(*step[1:]).wait_send()

    position = lax.axis_index("i")
    for chip in range(N_DEV):
        pl.when(position == chip)(lambda chip=chip: run(chip))


def pallas_dist_ring_attn_i_s256_d64_kernel(
    q: jax.Array,
    k: jax.Array,
    v: jax.Array,
):
    out_t = pl.pallas_call(
        _body,
        out_shape=jax.ShapeDtypeStruct((D, S_LOC), jnp.float32),
        in_specs=[pl.BlockSpec(memory_space=pltpu.HBM)] * 3,
        out_specs=pl.BlockSpec(memory_space=pltpu.VMEM),
        scratch_shapes=[
            pltpu.VMEM((3, D, S_LOC), jnp.float32),
            pltpu.VMEM((N_DEV, 2 * D, HALF), _BF16),
            pltpu.VMEM((N_DEV, 2 * D, HALF), _BF16),
            pltpu.SemaphoreType.DMA((max(len(m) for m in _LOAD_SEM),)),
            pltpu.SemaphoreType.DMA,
            pltpu.SemaphoreType.DMA((max(len(m) for m in _RECV_SEM),)),
            pltpu.SemaphoreType.REGULAR,
        ],
        compiler_params=pltpu.CompilerParams(collective_id=0, disable_semaphore_checks=True),
    )(q.T, k.T, v.T)
    return out_t.T
```

```python
import math

import jax
import jax.numpy as jnp
from jax import lax
from jax.experimental import pallas as pl
from jax.experimental.pallas import tpu as pltpu

N_DEV = 4
S_LOC = 256
D = 64
HALF = 128
_BF16 = jnp.bfloat16
_MESH = pl.DeviceIdType.MESH
_Q_SCALE = math.log2(math.e) / math.sqrt(D)

_LOADS = {
    "k": (0, None), "k0": (0, 0), "k1": (0, 1),
    "v": (1, None), "v0": (1, 0), "v1": (1, 1),
    "q": (2, None),
}

_PIECES = {
    "K": ("k", 0, 128), "K0": ("k", 0, 64), "K1": ("k", 64, 64),
    "V": ("v", 0, 128), "V0": ("v", 0, 64), "V1a": ("v", 64, 32), "V1b": ("v", 96, 32),
    "V0a": ("v", 0, 32),
}
_RELAY = ("R0", "R1", "R2", "R3", "R4", "R5")
_PIECES.update({name: ("v", start, 16) for name, start in zip(_RELAY, (64, 80, 96, 112, 32, 48))})


def _scores(block):
    return [("scores", block)]


def _values(*halves, last=False):
    return [("rescale", halves, last)] + [("pv",) + h for h in halves]


_PROGRAM = {
    0: (
        [("load", "k"), ("load", "v"), ("load", "q"), ("enter", (1, 3, 2)),
         ("use", "k"), ("entered", 2), ("send", "K", 0, 3), ("send", "K", 0, 1),
         ("use", "v"), ("send", "V", 0, 3), ("send", "V", 0, 1), ("use", "q")]
        + _scores(0) + _values((0, 0), (0, 1))
        + [("wait_go",), ("send", "K", 0, 2), ("send", "V", 0, 2),
           ("recv", "K", 3), ("send", "K", 3, 1), ("recv", "K0", 1), ("recv", "K1", 1)]
        + _scores(3) + _scores(1)
        + [("recv", "V", 3), ("send", "V", 3, 1), ("recv", "V0", 1)]
        + _values((3, 0), (3, 1), (1, 0))
        + [("recv", "K", 2)]
        + _scores(2)
        + [("recv", r, 2) for r in _RELAY[:4]] + [("recv", "V1a", 1), ("recv", "V1b", 1), ("recv", "V0a", 2)]
        + [("recv", r, 2) for r in _RELAY[4:]]
        + _values((2, 1), (2, 0), (1, 1), last=True)
        + [("store",)]
    ),
    1: (
        [("load", "k0"), ("load", "k1"), ("load", "v"), ("load", "q"), ("enter", (0, 2)),
         ("use", "k0"), ("entered", 1), ("send", "K0", 1, 0), ("use", "k1"), ("send", "K1", 1, 0),
         ("use", "v"), ("send", "V0", 1, 0), ("send", "V1a", 1, 0), ("use", "q")]
        + _scores(1) + _values((1, 0), (1, 1))
        + [("wait_go",), ("send", "K", 1, 3), ("send", "V", 1, 3), ("send", "K", 1, 2), ("send", "V", 1, 2),
           ("recv", "K", 0), ("send", "V1b", 1, 0)]
        + _scores(0) + [("recv", "V", 0)] + _values((0, 0), (0, 1))
        + [("recv", "K", 2)] + _scores(2) + [("recv", "K", 3)] + _scores(3)
        + [("recv", "V", 2)] + _values((2, 0), (2, 1))
        + [("recv", "V", 3)] + _values((3, 0), (3, 1), last=True)
        + [("store",)]
    ),
    2: (
        [("load", "v1"), ("load", "k"), ("load", "v0"), ("load", "q"),
         ("entered", 3), ("go", (1, 3, 0)),
         ("use", "v1")]
        + [("send", r, 2, 3) for r in _RELAY[:4]]
        + [("use", "k"), ("send", "K", 2, 0), ("use", "v0")]
        + [("send", r, 2, 3) for r in _RELAY[4:]]
        + [("send", "V0a", 2, 0),
           ("send", "K", 2, 3), ("send", "V0a", 2, 3), ("send", "K", 2, 1), ("send", "V", 2, 1), ("use", "q")]
        + _scores(2) + _values((2, 0), (2, 1))
        + [("recv", "K", 3)] + _scores(3) + [("recv", "V", 3)] + _values((3, 0), (3, 1))
        + [("recv", "K", 0)] + _scores(0) + [("recv", "K", 1)] + _scores(1)
        + [("recv", "V", 0)] + _values((0, 0), (0, 1))
        + [("recv", "V", 1)] + _values((1, 0), (1, 1), last=True)
        + [("store",)]
    ),
    3: (
        [("load", "k"), ("load", "v"), ("load", "q"), ("enter", (0, 2)),
         ("use", "k"), ("entered", 1), ("send", "K", 3, 0),
         ("use", "v"), ("send", "V", 3, 0), ("use", "q")]
        + _scores(3) + _values((3, 0), (3, 1))
        + [("wait_go",), ("send", "K", 3, 2), ("send", "V", 3, 2)]
        + [step for r in _RELAY for step in (("recv", r, 2), ("send", r, 2, 0))]
        + [("recv", "K", 0)] + _scores(0) + [("recv", "K", 2)] + _scores(2)
        + [("recv", "V", 0)] + _values((0, 0), (0, 1))
        + [("recv", "V0a", 2)] + _values((2, 0), (2, 1))
        + [("recv", "K", 1)] + _scores(1)
        + [("recv", "V", 1)] + _values((1, 0), (1, 1), last=True)
        + [("store",)]
    ),
}


def _semaphore_plan():
    recv, send, loads = [], [], []
    for chip in range(N_DEV):
        steps = _PROGRAM[chip]
        recv.append({s[1:]: n for n, s in enumerate(s for s in steps if s[0] == "recv")})
        send.append({s[1:]: n for n, s in enumerate(s for s in steps if s[0] == "send")})
        loads.append({s[1]: n for n, s in enumerate(s for s in steps if s[0] == "load")})
    sent = sorted(s[3:] + s[1:3] for chip in range(N_DEV) for s in _PROGRAM[chip] if s[0] == "send")
    received = sorted((chip,) + key for chip in range(N_DEV) for key in recv[chip])
    assert sent == received, "every remote copy needs exactly one matching wait"
    return recv, send, loads


_RECV_SEM, _SEND_SEM, _LOAD_SEM = _semaphore_plan()
_SENDER = {(s[3], s[1], s[2]): chip for chip in range(N_DEV) for s in _PROGRAM[chip] if s[0] == "send"}


def _body(q_hbm, k_hbm, v_hbm, o_ref, f32_buf, k_buf, v_buf, load_sems, send_sems, recv_sems, go_sem):
    hbm = (k_hbm, v_hbm, q_hbm)
    barrier = pltpu.get_barrier_semaphore()

    def piece(name, block):
        which, start, size = _PIECES[name]
        ref = (k_buf if which == "k" else v_buf).at[block]
        return ref if size == 2 * D else ref.at[pl.ds(start, size)]

    def run(me):
        def load(name):
            arr, half = _LOADS[name]
            src, dst = hbm[arr], f32_buf.at[arr]
            if half is not None:
                cols = pl.ds(half * HALF, HALF)
                src, dst = src.at[:, cols], dst.at[:, cols]
            return pltpu.make_async_copy(src, dst, load_sems.at[_LOAD_SEM[me][name]])

        def remote(name, block, src_chip, dst_chip):
            return pltpu.make_async_remote_copy(
                src_ref=piece(name, block),
                dst_ref=piece(name, block),
                send_sem=send_sems.at[_SEND_SEM[src_chip][(name, block, dst_chip)]],
                recv_sem=recv_sems.at[_RECV_SEM[dst_chip][(name, block)]],
                device_id=(dst_chip,),
                device_id_type=_MESH,
            )

        weights = None
        stats = {}
        scale = {}
        run_max = run_sum = acc = None
        for step in _PROGRAM[me]:
            kind = step[0]
            if kind == "load":
                load(step[1]).start()
            elif kind == "use":
                load(step[1]).wait()
                arr, half = _LOADS[step[1]]
                if arr == 2:
                    q_t = (f32_buf[2] * _Q_SCALE).astype(_BF16)
                    zero = jnp.zeros_like(q_t)
                    weights = (jnp.concatenate([q_t, zero], axis=0), jnp.concatenate([zero, q_t], axis=0))
                else:
                    dst = k_buf if arr == 0 else v_buf
                    for h in (0, 1) if half is None else (half,):
                        dst[me, h * D:(h + 1) * D] = f32_buf[arr, :, h * HALF:(h + 1) * HALF].astype(_BF16)
            elif kind == "enter":
                for chip in step[1]:
                    pl.semaphore_signal(barrier, inc=1, device_id=(chip,), device_id_type=_MESH)
            elif kind == "entered":
                pl.semaphore_wait(barrier, step[1])
            elif kind == "go":
                for chip in step[1]:
                    pl.semaphore_signal(go_sem, inc=1, device_id=(chip,), device_id_type=_MESH)
            elif kind == "wait_go":
                pl.semaphore_wait(go_sem, 1)
            elif kind == "send":
                remote(step[1], step[2], me, step[3]).start()
            elif kind == "recv":
                remote(step[1], step[2], _SENDER[(me,) + step[1:]], me).wait_recv()
            elif kind == "scores":
                keys = k_buf[step[1]].T
                for half in (0, 1):
                    s_t = jnp.dot(keys, weights[half], preferred_element_type=jnp.float32)
                    row_max = jnp.max(s_t, axis=0, keepdims=True)
                    p_t = jnp.exp2(s_t - row_max)
                    stats[(step[1], half)] = (row_max, jnp.sum(p_t, axis=0, keepdims=True), p_t.astype(_BF16))
            elif kind == "rescale":
                halves, last = step[1:]
                new_max = run_max
                for h in halves:
                    new_max = stats[h][0] if new_max is None else jnp.maximum(new_max, stats[h][0])
                for h in halves:
                    scale[h] = jnp.exp2(stats[h][0] - new_max)
                new_sum = None
                for h in halves:
                    term = stats[h][1] * scale[h]
                    new_sum = term if new_sum is None else new_sum + term
                if run_max is not None:
                    keep = jnp.exp2(run_max - new_max)
                    new_sum = new_sum + run_sum * keep
                if last:
                    inv_sum = 1.0 / new_sum
                    keep = keep * inv_sum
                    for h in halves:
                        scale[h] = scale[h] * inv_sum
                if acc is not None:
                    acc = acc * keep
                run_max, run_sum = new_max, new_sum
            elif kind == "pv":
                h = step[1:]
                v_t = v_buf[h[0], h[1] * D:(h[1] + 1) * D]
                out = jnp.dot(v_t, stats[h][2], preferred_element_type=jnp.float32) * scale[h]
                acc = out if acc is None else acc + out
            elif kind == "store":
                o_ref[...] = acc
            else:
                raise ValueError(step)
        for step in _PROGRAM[me]:
            if step[0] == "send":
                remote(step[1], step[2], me, step[3]).wait_send()

    position = lax.axis_index("i")
    for chip in range(N_DEV):
        pl.when(position == chip)(lambda chip=chip: run(chip))


def pallas_dist_ring_attn_i_s256_d64_kernel(
    q: jax.Array,
    k: jax.Array,
    v: jax.Array,
):
    out_t = pl.pallas_call(
        _body,
        out_shape=jax.ShapeDtypeStruct((D, S_LOC), jnp.float32),
        in_specs=[pl.BlockSpec(memory_space=pltpu.HBM)] * 3,
        out_specs=pl.BlockSpec(memory_space=pltpu.VMEM),
        scratch_shapes=[
            pltpu.VMEM((3, D, S_LOC), jnp.float32),
            pltpu.VMEM((N_DEV, 2 * D, HALF), _BF16),
            pltpu.VMEM((N_DEV, 2 * D, HALF), _BF16),
            pltpu.SemaphoreType.DMA((max(len(m) for m in _LOAD_SEM),)),
            pltpu.SemaphoreType.DMA((max(len(m) for m in _SEND_SEM),)),
            pltpu.SemaphoreType.DMA((max(len(m) for m in _RECV_SEM),)),
            pltpu.SemaphoreType.REGULAR,
        ],
        compiler_params=pltpu.CompilerParams(collective_id=0, disable_semaphore_checks=True),
    )(q.T, k.T, v.T)
    return out_t.T
```
